```python
import numpy as np

kernel_name = "dist_rsx_agy_m2048_n1024"

def setup_inputs():
    return {"x": np.random.randn(2, 2048, 2048).astype(np.float32)}

def reference(x: np.ndarray) -> np.ndarray:
    return x.sum(axis=0)
```

```python
import functools
import jax
import jax.numpy as jnp
from jax import lax
from jax.experimental import pallas as pl
from jax.experimental.pallas import tpu as pltpu
MESH = pl.DeviceIdType.MESH
M, N = 2048, 1024

def make(R=32, D=4, E=2, K=8, LD=2, out_dtype=jnp.float32, nocheck=False, unroll=True, outmode='sds_hbm', vlim=100):
    n = M // R
    def fn(x):
        def body(x_ref, o_ref, xin, xs, xr, ys, yr, own, oth, lsem, xrs, yrs, ssem, osem):
            mx, my = lax.axis_index("x"), lax.axis_index("y")
            nx, ny = (1 - mx, my), (mx, 1 - my)
            NL = D + LD
            rows = lambda c: pl.ds(c * R if isinstance(c, int) else pl.multiple_of(c * R, R), R)
            mycols = pl.ds(pl.multiple_of(my * N, N), N)
            otcols = pl.ds(pl.multiple_of((1 - my) * N, N), N)
            load = lambda c: pltpu.make_async_copy(x_ref.at[0, rows(c)], xin.at[rows(c)], lsem.at[c % NL])
            xsend = lambda c: pltpu.make_async_remote_copy(xs.at[rows(c)], xr.at[rows(c)], ssem, xrs.at[c % K], device_id=nx, device_id_type=MESH)
            ysend = lambda c: pltpu.make_async_remote_copy(ys.at[rows(c)], yr.at[rows(c)], ssem, yrs.at[c % K], device_id=ny, device_id_type=MESH)
            st_own = lambda c: pltpu.make_async_copy(own.at[rows(c)], o_ref.at[rows(c), mycols], osem)
            st_oth = lambda c: pltpu.make_async_copy(oth.at[rows(c)], o_ref.at[rows(c), otcols], osem)

            for c in range(NL):
                load(c).start()
            b = pltpu.get_barrier_semaphore()
            for nb in (nx, ny):
                pl.semaphore_signal(b, inc=1, device_id=nb, device_id_type=MESH)

            def stage1(c, first=False, more=True):
                load(c).wait()
                xs[rows(c), :] = xin[rows(c), :].astype(jnp.bfloat16)
                if first:
                    pl.semaphore_wait(b, 2)
                xsend(c).start()
                if more:
                    load(c + NL).start()
            def stage2(c):
                xsend(c).wait_recv()
                s = (xs[rows(c), :].astype(jnp.float32) + xr[rows(c), :].astype(jnp.float32)).astype(jnp.bfloat16)
                ys[rows(c), :] = s
                ysend(c).start()
                own[rows(c), :] = s.astype(out_dtype)
                st_own(c).start()
            def stage3(c):
                ysend(c).wait_recv()
                oth[rows(c), :] = yr[rows(c), :].astype(out_dtype)
                st_oth(c).start()

            for c in range(D):
                stage1(c, first=(c == 0))
            if unroll:
                for i in range(n + E):
                    if i < n:
                        stage2(i)
                    if i + D < n:
                        stage1(i + D, more=(i + D + NL < n))
                    if i - E >= 0:
                        stage3(i - E)
            else:
                for i in range(E):
                    stage2(i); stage1(i + D)
                hi = n - D - NL
                def step(i, _):
                    stage2(i); stage1(i + D); stage3(i - E)
                    return _
                lax.fori_loop(E, hi, step, 0)
                for i in range(hi, n + E):
                    if i < n:
                        stage2(i)
                    if i + D < n:
                        stage1(i + D, more=False)
                    stage3(i - E)
            pltpu.make_async_copy(xs, xs, ssem).wait()
            pltpu.make_async_copy(ys, ys, ssem).wait()
            pltpu.make_async_copy(own, own, osem).wait()
            pltpu.make_async_copy(oth, oth, osem).wait()
        return pl.pallas_call(
            body, out_shape=(pltpu.HBM((M, 2 * N), out_dtype) if outmode=='hbm' else jax.ShapeDtypeStruct((M, 2 * N), out_dtype)),
            in_specs=[pl.BlockSpec(memory_space=pltpu.HBM)],
            out_specs=pl.BlockSpec(memory_space=(pl.ANY if outmode=='any' else pltpu.HBM)),
            scratch_shapes=[pltpu.VMEM((M, N), jnp.float32)] + [pltpu.VMEM((M, N), jnp.bfloat16)] * 4
              + [pltpu.VMEM((M, N), out_dtype)] * 2
              + [pltpu.SemaphoreType.DMA((D + LD,)), pltpu.SemaphoreType.DMA((K,)), pltpu.SemaphoreType.DMA((K,)),
                 pltpu.SemaphoreType.DMA, pltpu.SemaphoreType.DMA],
            compiler_params=pltpu.CompilerParams(collective_id=0, vmem_limit_bytes=vlim << 20, disable_semaphore_checks=nocheck),
            name="base1",
        )(x)
    return fn


def pallas_dist_rsx_agy_m2048_n1024_kernel(x):
    return make(R=16, D=4, unroll=False, outmode="any", vlim=100)(x)
```

```python
import functools
import jax
import jax.numpy as jnp
from jax import lax
from jax.experimental import pallas as pl
from jax.experimental.pallas import tpu as pltpu
MESH = pl.DeviceIdType.MESH
M, N = 2048, 1024
bf = jnp.bfloat16

def make(R=16, D=4, E=2, K=8, LD=2, nocheck=False, unroll=False, custom_barrier=True):
    n = M // R
    def fn(x):
        def body(x_ref, o_ref, xin, xs, xr, lsem, xrs, yrs, ssem):
            mx, my = lax.axis_index("x"), lax.axis_index("y")
            nx, ny = (1 - mx, my), (mx, 1 - my)
            NL = D + LD
            rows = lambda c: pl.ds(c * R if isinstance(c, int) else pl.multiple_of(c * R, R), R)
            mycols = pl.ds(pl.multiple_of(my * N, N), N)
            load = lambda c: pltpu.make_async_copy(x_ref.at[0, rows(c)], xin.at[rows(c)], lsem.at[c % NL])
            xsend = lambda c: pltpu.make_async_remote_copy(xs.at[rows(c)], xr.at[rows(c)], ssem, xrs.at[c % K], device_id=nx, device_id_type=MESH)
            ysend = lambda c: pltpu.make_async_remote_copy(o_ref.at[rows(c), mycols], o_ref.at[rows(c), mycols], ssem, yrs.at[c % K], device_id=ny, device_id_type=MESH)

            for c in range(NL):
                load(c).start()
            if custom_barrier:
                b = pltpu.get_barrier_semaphore()
                for nb in (nx, ny):
                    pl.semaphore_signal(b, inc=1, device_id=nb, device_id_type=MESH)

            def stage1(c, first=False, more=True):
                load(c).wait()
                xs[rows(c), :] = xin[rows(c), :].astype(bf)
                if first and custom_barrier:
                    pl.semaphore_wait(b, 2)
                xsend(c).start()
                if more:
                    load(c + NL).start()
            def stage2(c):
                xsend(c).wait_recv()
                s = (xs[rows(c), :].astype(jnp.float32) + xr[rows(c), :].astype(jnp.float32)).astype(bf)
                o_ref[rows(c), mycols] = s
                ysend(c).start()
            def stage3(c):
                ysend(c).wait_recv()

            for c in range(D):
                stage1(c, first=(c == 0))
            if unroll:
                for i in range(n + E):
                    if i < n:
                        stage2(i)
                    if i + D < n:
                        stage1(i + D, more=(i + D + NL < n))
                    if i - E >= 0:
                        stage3(i - E)
            else:
                for i in range(E):
                    stage2(i); stage1(i + D)
                hi = n - D - NL
                def step(i, _):
                    stage2(i); stage1(i + D); stage3(i - E)
                    return _
                lax.fori_loop(E, hi, step, 0)
                for i in range(hi, n + E):
                    if i < n:
                        stage2(i)
                    if i + D < n:
                        stage1(i + D, more=False)
                    stage3(i - E)
            pltpu.make_async_copy(xs, xs, ssem).wait()
            pltpu.make_async_copy(xs, xs, ssem).wait()
        return pl.pallas_call(
            body, out_shape=pltpu.VMEM((M, 2 * N), bf),
            in_specs=[pl.BlockSpec(memory_space=pltpu.HBM)],
            out_specs=pl.BlockSpec(memory_space=pltpu.VMEM),
            scratch_shapes=[pltpu.VMEM((M, N), jnp.float32)] + [pltpu.VMEM((M, N), bf)] * 2
              + [pltpu.SemaphoreType.DMA((D + LD,)), pltpu.SemaphoreType.DMA((K,)), pltpu.SemaphoreType.DMA((K,)),
                 pltpu.SemaphoreType.DMA],
            compiler_params=pltpu.CompilerParams(collective_id=0 if custom_barrier else None, vmem_limit_bytes=32 << 20, disable_semaphore_checks=nocheck),
            name="base2",
        )(x)
    return fn


def pallas_dist_rsx_agy_m2048_n1024_kernel(x):
    return make(R=16, D=4)(x)
```

```python
import jax
import jax.numpy as jnp
from jax import lax
from jax.experimental import pallas as pl
from jax.experimental.pallas import tpu as pltpu

I32, F32, BF16 = jnp.int32, jnp.float32, jnp.bfloat16
TILE = (8, 128)
ROWS = 32

MAIN_ROWS = 90
EXTRA_AT, EXTRA_ROWS = 96, 40
SLOT_ROWS = 160

AHEAD = 3
LAG = 3
RING = 8
LOADS = 4
assert RING >= 2 * AHEAD and RING >= 2 * LAG + 2


def _bytes(b):
    v = b * 0x01010101
    return v - (1 << 32) if v >= 1 << 31 else v


def _shr(x, n):
    return lax.shift_right_logical(x, jnp.full_like(x, n) if isinstance(n, int) else n)


def _rotl(x, n):
    return (x << n) | _shr(x, 32 - n)


def _over_sublanes(op, x):
    for s in (4, 2, 1):
        x = op(x, pltpu.roll(x, s, 0))
    return x


def _sublane_cumsum(x):
    sublane = lax.broadcasted_iota(I32, TILE, 0)
    for s in (1, 2, 4):
        x = x + jnp.where(sublane >= s, pltpu.roll(x, s, 0), 0)
    return x


def _is_plain(head):
    return _shr(head, 24) == 255


def _encode(words):
    rest, exps, top = [], [], None
    for a, b in zip(words[:8], words[8:]):
        a, b = _rotl(a, 1), _rotl(b, 1)
        swap = (_shr(a, 8) ^ b) & 0x00FF00FF
        e = b ^ swap
        exps.append(e)
        rest.append(a ^ (swap << 8))
        p, q = e & 0x00FF00FF, _shr(e, 8) & 0x00FF00FF
        m = jnp.maximum(jnp.maximum(p, q), jnp.maximum(p << 16, q << 16))
        top = m if top is None else jnp.maximum(top, m)
    top = _shr(_over_sublanes(jnp.maximum, top), 16)

    codes = []
    string = length = seen = jnp.zeros(TILE, I32)
    for e in exps:
        g = top * _bytes(1) - e
        s = g + _bytes(0x80 - 7)
        escape = s & _bytes(0x80)
        mask = _shr(escape, 2) - _shr(escape, 7)
        unary = (s + _bytes(1)) & mask
        for n in (unary & 255, _shr(unary, 8) & 255, _shr(unary, 16) & 255, _shr(unary, 24)):
            string = (string << n) | jnp.minimum(n, 1)
        length = length + unary
        seen = seen | g
        codes.append(g | mask)

    length = (length & 0x00FF00FF) + (_shr(length, 8) & 0x00FF00FF)
    length = (length & 0xFFFF) + _shr(length, 16)
    end = _sublane_cumsum(length) + 8
    too_long = (length > 32) | (end > 64) | ((seen & _bytes(0xE0)) != 0)
    shift = jnp.maximum(64 - end, 0)
    s = shift & 31
    head0 = jnp.where(shift >= 32, string << s, _shr(_shr(string, 1), 31 - s)) & 0x00FFFFFF
    head1 = jnp.where(shift >= 32, 0, string << s)
    head0 = _over_sublanes(jnp.bitwise_or, jnp.where(too_long, -1, head0)) | (top << 24)
    head1 = _over_sublanes(jnp.bitwise_or, head1)

    plain = _is_plain(head0)
    c = [jnp.where(plain, e, k) & _bytes(7) for e, k in zip(exps, codes)]
    packed = [
        c[0] | (c[1] << 3) | ((c[6] & _bytes(3)) << 6),
        c[2] | (c[3] << 3) | ((c[7] & _bytes(3)) << 6),
        c[4] | (c[5] << 3) | ((c[6] & _bytes(4)) << 4) | ((c[7] & _bytes(4)) << 5),
    ]
    head = jnp.where(lax.broadcasted_iota(I32, TILE, 0) == 0, head0, head1)
    return rest + packed + [head], exps


def _pack_extra(exps):
    nibbles = [
        (_shr(exps[j], 3) & _bytes(0x0F)) | ((exps[j + 1] << 1) & _bytes(0xF0))
        for j in range(0, 8, 2)
    ]
    high = exps[0] & _bytes(0x80)
    for j in range(1, 8):
        high = high | _shr(exps[j] & _bytes(0x80), j)
    return nibbles + [high]


def _unpack_extra(tiles):
    return [
        ((_shr(tiles[j // 2], 1) if j % 2 else tiles[j // 2] << 3) & _bytes(0x78))
        | ((tiles[4] << j) & _bytes(0x80))
        for j in range(8)
    ]


def _decode(rest, packed, head0, head1, extra):
    p0, p1, p2 = packed
    codes = [
        p0 & _bytes(7), _shr(p0, 3) & _bytes(7),
        p1 & _bytes(7), _shr(p1, 3) & _bytes(7),
        p2 & _bytes(7), _shr(p2, 3) & _bytes(7),
        (_shr(p0, 6) & _bytes(3)) | (_shr(p2, 4) & _bytes(4)),
        (_shr(p1, 6) & _bytes(3)) | (_shr(p2, 5) & _bytes(4)),
    ]
    escapes = [(k + _bytes(1)) & _bytes(8) for k in codes]

    count = _shr(_shr(sum(escapes[1:], escapes[0]), 3) * _bytes(1), 24)
    skip = _sublane_cumsum(count) - count
    first = head0 & 0x00FFFFFF
    ones = lax.population_count(first)
    second = skip > ones
    window = jnp.where(second, head1, first)
    left = jnp.where(second, skip - ones, skip)
    start = jnp.where(second, 33, 1)
    for step in (16, 8, 4, 2, 1):
        ones = lax.population_count(_shr(window, 32 - step))
        advance = ones < left
        window = jnp.where(advance, window << step, window)
        left = jnp.where(advance, left - ones, left)
        start = jnp.where(advance, start + step, start)
    start = jnp.where(skip == 0, 8, start)
    s = start & 31
    string = jnp.where(start >= 32, head1 << s, (head0 << s) | _shr(_shr(head1, 1), 31 - s))

    top = _shr(head0, 24) * _bytes(1)
    a, b = [], []
    for j in range(8):
        one = _shr(escapes[j], 3)
        mask = (escapes[j] << 2) - one
        g = codes[j] - one
        for byte in range(4):
            n = (lax.clz(string) + 1) & (_shr(mask, 8 * byte) if byte else mask)
            string = string << n
            g = g + (n << (8 * byte) if byte else n)
        e = top - g
        if extra is not None:
            e = jnp.where(_is_plain(head0), codes[j] | extra[j], e)
        swap = (e ^ _shr(rest[j], 8)) & 0x00FF00FF
        a.append(_rotl(rest[j] ^ (swap << 8), 31))
        b.append(_rotl(e ^ swap, 31))
    return a + b


def _pairs(block):
    def tile(i, j):
        return block[8 * i:8 * i + 8, 128 * j:128 * j + 128]

    return [(tile(i, j), tile(i + 1, j)) for i in (0, 2) for j in range(8)]


def _add(u, v):
    return [(a + c, b + d) for (a, b), (c, d) in zip(u, v)]


def _read_tiles(msg, lo, hi):
    return [msg[8 * j:8 * j + 8, :] for j in range(lo, hi)]


def _write_tiles(msg, lo, tiles):
    for j, t in enumerate(tiles, lo):
        msg[8 * j:8 * j + 8, :] = t


def _header(msg, k=0):
    return jnp.broadcast_to(msg[88 + k:89 + k, :], TILE)


def _write_message(msg, pairs):
    words = [
        lax.bitcast_convert_type(pltpu.pack_elementwise(list(p), packed_dtype=BF16), I32)
        for p in pairs
    ]
    main, exps = _encode(words)
    _write_tiles(msg, 0, main + exps)


def _read_message(msg, with_extra):
    extra = _unpack_extra(_read_tiles(msg, 12, 17)) if with_extra else None
    words = _decode(
        _read_tiles(msg, 0, 8), _read_tiles(msg, 8, 11), _header(msg, 0), _header(msg, 1), extra
    )
    return [
        tuple(lax.bitcast_convert_type(h, F32) for h in (w << 16, w & -65536)) for w in words
    ]


def _needs_extra(msgs):
    sublane = lax.broadcasted_iota(I32, TILE, 0)
    bits = jnp.zeros(TILE, F32)
    for k, msg in enumerate(msgs):
        bits = jnp.where((sublane == k) & _is_plain(_header(msg)), float(1 << k), bits)
    bits = jnp.sum(jnp.max(bits, axis=1, keepdims=True), axis=0, keepdims=True)
    return bits.astype(I32)[0, 0]


def _body(x_ref, o_ref, block, send, recv, gathered, flag,
          load_sem, main_sem, extra_sem, gather_sem, sent_main_sem, sent_extra_sem):
    n = block.shape[0]
    cols = x_ref.shape[2]
    last = n - 1
    mx, my = lax.axis_index("x"), lax.axis_index("y")
    neighbour = ((1 - mx, my), (mx, 1 - my))
    mine = pl.ds(pl.multiple_of(my * cols, cols), cols)
    other = pl.ds(pl.multiple_of((1 - my) * cols, cols), cols)

    def rows(c):
        return pl.ds(c * ROWS if isinstance(c, int) else pl.multiple_of(c * ROWS, ROWS), ROWS)

    def load(c, sem=None):
        sem = load_sem.at[c & (LOADS - 1)] if sem is None else sem
        return pltpu.make_async_copy(x_ref.at[0, rows(c)], block.at[c], sem)

    def store(c, where, pairs):
        tiles = [[p[h] for p in pairs[k:k + 8]] for k in (0, 8) for h in (0, 1)]
        whole = jnp.concatenate([jnp.concatenate(r, axis=1) for r in tiles], axis=0)
        o_ref[rows(c), where] = whole.astype(BF16)

    class Message:
        def __init__(self, src, dst, link, main, extra):
            self.src, self.dst, self.link, self.sems = src, dst, link, (main, extra)

        def _copy(self, part, send_sem, recv_sem):
            return pltpu.make_async_remote_copy(
                self.src.at[part], self.dst.at[part], send_sem, recv_sem,
                device_id=neighbour[self.link], device_id_type=pl.DeviceIdType.MESH)

        def main(self):
            return self._copy(pl.ds(0, MAIN_ROWS), sent_main_sem.at[self.link], self.sems[0])

        def extra(self):
            return self._copy(pl.ds(EXTRA_AT, EXTRA_ROWS), sent_extra_sem, self.sems[1])

        def send_extra(self):
            _write_tiles(self.src, 12, _pack_extra(_read_tiles(self.src, 12, 20)))
            self.extra().start()

        def receive(self, use):
            self.main().wait_recv()
            more = _needs_extra([self.dst])
            use(_read_message(self.dst, False))

            @pl.when(more != 0)
            def _():
                self.extra().wait_recv()
                use(_read_message(self.dst, True))

            return more

    def streamed(link, c):
        slot = c & (RING - 1)
        return Message(send.at[link, c], recv.at[link, c], link,
                       main_sem.at[link, slot], extra_sem.at[link, slot])

    gather = Message(send.at[0, last], recv.at[1, last], 1, gather_sem.at[0], gather_sem.at[1])
    slot = n & (RING - 1)
    pass_on = Message(recv.at[1, last], recv.at[0, n], 0,
                      main_sem.at[0, slot], extra_sem.at[0, slot])

    for c in range(LOADS):
        load(c).start()
    load(last, load_sem.at[LOADS]).start()
    barrier = pltpu.get_barrier_semaphore()
    for peer in neighbour:
        pl.semaphore_signal(barrier, inc=1, device_id=peer, device_id_type=pl.DeviceIdType.MESH)

    def lead_in(c, extras):
        msg = streamed(0, c)
        load(c).wait()
        _write_message(msg.src, _pairs(block.at[c]))
        pl.when(c == 0)(lambda: pl.semaphore_wait(barrier, 2))
        msg.main().start()
        load(c + LOADS).start()
        more = _needs_extra([msg.src])
        pl.when(more != 0)(msg.send_extra)
        return extras + more

    extras = lax.fori_loop(0, AHEAD, lead_in, 0)

    load(last, load_sem.at[LOADS]).wait()
    _write_message(gather.src, _pairs(block.at[last]))
    gather.main().start()
    last_more = _needs_extra([gather.src])
    pl.when(last_more != 0)(gather.send_extra)
    extras = extras + 2 * last_more

    def step(i, extras):
        unpacking = i >= LAG
        j = jnp.maximum(i - LAG, 0)
        addend, summed, theirs = streamed(0, i), streamed(1, i), streamed(1, j)
        sent_x = streamed(0, jnp.minimum(i + AHEAD - 1, last - 1))
        sent_y = streamed(1, jnp.maximum(i - 1, 0))

        pl.when(unpacking)(lambda: theirs.main().wait_recv())
        addend.main().wait_recv()
        more = _needs_extra([
            addend.dst,
            recv.at[unpacking.astype(I32), jnp.where(unpacking, j, i)],
            sent_x.src,
            send.at[(i > 0).astype(I32), jnp.maximum(i - 1, 0)],
        ])
        more_x = ((more & 4) != 0) & (i > 0) & (i + AHEAD - 1 < last)
        more_y = ((more & 8) != 0) & (i > 0)

        def add(with_extra):
            total = _add(_pairs(block.at[i]), _read_message(addend.dst, with_extra))
            _write_message(summed.src, total)
            store(i, mine, total)

        add(False)

        @pl.when(more != 0)
        def _():
            pl.when(more_x)(sent_x.send_extra)
            pl.when(more_y)(sent_y.send_extra)

            @pl.when((more & 1) != 0)
            def _():
                addend.extra().wait_recv()
                add(True)

        summed.main().start()

        c = i + AHEAD

        @pl.when(c < last)
        def _():
            load(c).wait()
            _write_message(send.at[0, c], _pairs(block.at[c]))
            streamed(0, c).main().start()
            pl.when(c + LOADS < last)(lambda: load(c + LOADS).start())

        @pl.when(c == last)
        def _():
            streamed(0, last).main().start()
            pl.when(last_more != 0)(lambda: streamed(0, last).extra().start())

        @pl.when(c == n)
        def _():
            pass_on.main().start()
            pl.when(flag[0] != 0)(lambda: pass_on.extra().start())

        @pl.when(i == LAG - 1)
        def _():
            def keep(pairs):
                _write_tiles(gathered, 0, [t for p in pairs for t in p])

            flag[0] = gather.receive(keep)

        @pl.when(unpacking)
        def _():
            store(j, other, _read_message(theirs.dst, False))

            @pl.when((more & 2) != 0)
            def _():
                theirs.extra().wait_recv()
                store(j, other, _read_message(theirs.dst, True))

        return extras + more_x.astype(I32) + more_y.astype(I32)

    extras = lax.fori_loop(0, last, step, extras) + flag[0]
    more = _needs_extra([streamed(1, last - 1).src])
    pl.when(more != 0)(streamed(1, last - 1).send_extra)
    extras = extras + more

    def unpack(j):
        streamed(1, j).receive(lambda v: store(j, other, v))

    for j in range(last - LAG, last - 2):
        unpack(j)
    streamed(0, last).receive(lambda v: store(last, mine, _add(_pairs(block.at[last]), v)))
    unpack(last - 2)

    def finish(v):
        t = _read_tiles(gathered, 0, 32)
        store(last, other, _add(zip(t[0::2], t[1::2]), v))

    pass_on.receive(finish)
    unpack(last - 1)

    def wait_sent(src, sem):
        pltpu.make_async_remote_copy(
            src, src, sem, sem, device_id=neighbour[0],
            device_id_type=pl.DeviceIdType.MESH).wait_send()

    wait_sent(send.at[0, :, pl.ds(0, MAIN_ROWS)], sent_main_sem.at[0])
    wait_sent(send.at[1, pl.ds(0, n), pl.ds(0, MAIN_ROWS)], sent_main_sem.at[1])

    @pl.loop(0, extras)
    def _(_):
        wait_sent(send.at[0, 0, pl.ds(EXTRA_AT, EXTRA_ROWS)], sent_extra_sem)


def pallas_dist_rsx_agy_m2048_n1024_kernel(x: jax.Array):
    _, m, cols = x.shape
    n = m // ROWS
    messages = pltpu.VMEM((2, n + 1, SLOT_ROWS, 128), I32)
    return pl.pallas_call(
        _body,
        out_shape=pltpu.VMEM((m, 2 * cols), BF16),
        in_specs=[pl.BlockSpec(memory_space=pltpu.HBM)],
        out_specs=pl.BlockSpec(memory_space=pltpu.VMEM),
        scratch_shapes=[
            pltpu.VMEM((n, ROWS, cols), F32),
            messages,
            messages,
            pltpu.VMEM((256, 128), F32),
            pltpu.SMEM((1,), I32),
            pltpu.SemaphoreType.DMA((LOADS + 1,)),
            pltpu.SemaphoreType.DMA((2, RING)),
            pltpu.SemaphoreType.DMA((2, RING)),
            pltpu.SemaphoreType.DMA((2,)),
            pltpu.SemaphoreType.DMA((2,)),
            pltpu.SemaphoreType.DMA,
        ],
        compiler_params=pltpu.CompilerParams(
            collective_id=0, vmem_limit_bytes=40 << 20, disable_semaphore_checks=True),
        name="rsx_agy",
    )(x)
```

```python
import jax
import jax.numpy as jnp
from jax import lax
from jax.experimental import pallas as pl
from jax.experimental.pallas import tpu as pltpu

I32, F32, BF16 = jnp.int32, jnp.float32, jnp.bfloat16
TILE = (8, 128)
ROWS = 32

MAIN_ROWS = 90
EXTRA_AT, EXTRA_ROWS = 96, 40
SLOT_ROWS = 160

AHEAD = 3
LAG = 3
RING = 8
LOADS = 4
assert RING >= 2 * AHEAD and RING >= 2 * LAG + 2


def _bytes(b):
    v = b * 0x01010101
    return v - (1 << 32) if v >= 1 << 31 else v


def _shr(x, n):
    return lax.shift_right_logical(x, jnp.full_like(x, n) if isinstance(n, int) else n)


def _rotl(x, n):
    return (x << n) | _shr(x, 32 - n)


def _over_sublanes(op, x):
    for s in (4, 2, 1):
        x = op(x, pltpu.roll(x, s, 0))
    return x


def _sublane_cumsum(x):
    sublane = lax.broadcasted_iota(I32, TILE, 0)
    for s in (1, 2, 4):
        x = x + jnp.where(sublane >= s, pltpu.roll(x, s, 0), 0)
    return x


def _is_plain(head):
    return _shr(head, 24) == 255


def _encode(words):
    rest, exps, top = [], [], None
    for a, b in zip(words[:8], words[8:]):
        a, b = _rotl(a, 1), _rotl(b, 1)
        swap = (_shr(a, 8) ^ b) & 0x00FF00FF
        e = b ^ swap
        exps.append(e)
        rest.append(a ^ (swap << 8))
        p, q = e & 0x00FF00FF, _shr(e, 8) & 0x00FF00FF
        m = jnp.maximum(jnp.maximum(p, q), jnp.maximum(p << 16, q << 16))
        top = m if top is None else jnp.maximum(top, m)
    top = _shr(_over_sublanes(jnp.maximum, top), 16)

    codes = []
    string = length = seen = jnp.zeros(TILE, I32)
    for e in exps:
        g = top * _bytes(1) - e
        s = g + _bytes(0x80 - 7)
        escape = s & _bytes(0x80)
        mask = _shr(escape, 2) - _shr(escape, 7)
        unary = (s + _bytes(1)) & mask
        for n in (unary & 255, _shr(unary, 8) & 255, _shr(unary, 16) & 255, _shr(unary, 24)):
            string = (string << n) | jnp.minimum(n, 1)
        length = length + unary
        seen = seen | g
        codes.append(g | mask)

    length = (length & 0x00FF00FF) + (_shr(length, 8) & 0x00FF00FF)
    length = (length & 0xFFFF) + _shr(length, 16)
    end = _sublane_cumsum(length) + 8
    too_long = (length > 32) | (end > 64) | ((seen & _bytes(0xE0)) != 0)
    shift = jnp.maximum(64 - end, 0)
    s = shift & 31
    head0 = jnp.where(shift >= 32, string << s, _shr(_shr(string, 1), 31 - s)) & 0x00FFFFFF
    head1 = jnp.where(shift >= 32, 0, string << s)
    head0 = _over_sublanes(jnp.bitwise_or, jnp.where(too_long, -1, head0)) | (top << 24)
    head1 = _over_sublanes(jnp.bitwise_or, head1)

    plain = _is_plain(head0)
    c = [jnp.where(plain, e, k) & _bytes(7) for e, k in zip(exps, codes)]
    packed = [
        c[0] | (c[1] << 3) | ((c[6] & _bytes(3)) << 6),
        c[2] | (c[3] << 3) | ((c[7] & _bytes(3)) << 6),
        c[4] | (c[5] << 3) | ((c[6] & _bytes(4)) << 4) | ((c[7] & _bytes(4)) << 5),
    ]
    head = jnp.where(lax.broadcasted_iota(I32, TILE, 0) == 0, head0, head1)
    return rest + packed + [head], exps


def _pack_extra(exps):
    nibbles = [
        (_shr(exps[j], 3) & _bytes(0x0F)) | ((exps[j + 1] << 1) & _bytes(0xF0))
        for j in range(0, 8, 2)
    ]
    high = exps[0] & _bytes(0x80)
    for j in range(1, 8):
        high = high | _shr(exps[j] & _bytes(0x80), j)
    return nibbles + [high]


def _unpack_extra(tiles):
    return [
        ((_shr(tiles[j // 2], 1) if j % 2 else tiles[j // 2] << 3) & _bytes(0x78))
        | ((tiles[4] << j) & _bytes(0x80))
        for j in range(8)
    ]


def _decode(rest, packed, head0, head1, extra):
    p0, p1, p2 = packed
    codes = [
        p0 & _bytes(7), _shr(p0, 3) & _bytes(7),
        p1 & _bytes(7), _shr(p1, 3) & _bytes(7),
        p2 & _bytes(7), _shr(p2, 3) & _bytes(7),
        (_shr(p0, 6) & _bytes(3)) | (_shr(p2, 4) & _bytes(4)),
        (_shr(p1, 6) & _bytes(3)) | (_shr(p2, 5) & _bytes(4)),
    ]
    escapes = [(k + _bytes(1)) & _bytes(8) for k in codes]

    def count(es):
        return _shr(_shr(sum(es[1:], es[0]), 3) * _bytes(1), 24)

    def string_after(skip):
        first = head0 & 0x00FFFFFF
        ones = lax.population_count(first)
        second = skip > ones
        window = jnp.where(second, head1, first)
        left = jnp.where(second, skip - ones, skip)
        start = jnp.where(second, 33, 1)
        for step in (16, 8, 4, 2, 1):
            ones = lax.population_count(_shr(window, 32 - step))
            advance = ones < left
            window = jnp.where(advance, window << step, window)
            left = jnp.where(advance, left - ones, left)
            start = jnp.where(advance, start + step, start)
        start = jnp.where(skip == 0, 8, start)
        s = start & 31
        return jnp.where(start >= 32, head1 << s, (head0 << s) | _shr(_shr(head1, 1), 31 - s))

    early, late = count(escapes[:4]), count(escapes[4:])
    end = _sublane_cumsum(early + late)
    strings = {0: string_after(end - late - early), 4: string_after(end - late)}

    top = _shr(head0, 24) * _bytes(1)
    a, b = [], []
    for j in range(8):
        string = strings.get(j, string if j else None)
        one = _shr(escapes[j], 3)
        mask = (escapes[j] << 2) - one
        g = codes[j] - one
        for byte in range(4):
            n = (lax.clz(string) + 1) & (_shr(mask, 8 * byte) if byte else mask)
            string = string << n
            g = g + (n << (8 * byte) if byte else n)
        e = top - g
        if extra is not None:
            e = jnp.where(_is_plain(head0), codes[j] | extra[j], e)
        swap = (e ^ _shr(rest[j], 8)) & 0x00FF00FF
        a.append(_rotl(rest[j] ^ (swap << 8), 31))
        b.append(_rotl(e ^ swap, 31))
    return a + b


def _pieces(block):
    return [block[i:i + 16, j:j + 128] for i in (0, 16) for j in range(0, 1024, 128)]


def _add(u, v):
    return [a + b for a, b in zip(u, v)]


def _read_tiles(msg, lo, hi):
    return [msg[8 * j:8 * j + 8, :] for j in range(lo, hi)]


def _write_tiles(msg, lo, tiles):
    for j, t in enumerate(tiles, lo):
        msg[8 * j:8 * j + 8, :] = t


def _header(msg, k=0):
    return jnp.broadcast_to(msg[88 + k:89 + k, :], TILE)


def _write_message(msg, pieces):
    main, exps = _encode([pltpu.bitcast(p.astype(BF16), I32) for p in pieces])
    _write_tiles(msg, 0, main + exps)


def _read_message(msg, with_extra):
    extra = _unpack_extra(_read_tiles(msg, 12, 17)) if with_extra else None
    words = _decode(
        _read_tiles(msg, 0, 8), _read_tiles(msg, 8, 11), _header(msg, 0), _header(msg, 1), extra
    )
    return [pltpu.bitcast(w, BF16).astype(F32) for w in words]


def _needs_extra(msgs):
    sublane = lax.broadcasted_iota(I32, TILE, 0)
    bits = jnp.zeros(TILE, F32)
    for k, msg in enumerate(msgs):
        bits = jnp.where((sublane == k) & _is_plain(_header(msg)), float(1 << k), bits)
    bits = jnp.sum(jnp.max(bits, axis=1, keepdims=True), axis=0, keepdims=True)
    return bits.astype(I32)[0, 0]


def _body(x_ref, o_ref, block, send, recv, gathered, flag,
          load_sem, main_sem, extra_sem, gather_sem, sent_main_sem, sent_extra_sem):
    n = block.shape[0]
    cols = x_ref.shape[2]
    last = n - 1
    mx, my = lax.axis_index("x"), lax.axis_index("y")
    neighbour = ((1 - mx, my), (mx, 1 - my))
    mine = pl.ds(pl.multiple_of(my * cols, cols), cols)
    other = pl.ds(pl.multiple_of((1 - my) * cols, cols), cols)

    def rows(c):
        return pl.ds(c * ROWS if isinstance(c, int) else pl.multiple_of(c * ROWS, ROWS), ROWS)

    def load(c, sem=None):
        sem = load_sem.at[c & (LOADS - 1)] if sem is None else sem
        return pltpu.make_async_copy(x_ref.at[0, rows(c)], block.at[c], sem)

    def joined(pieces):
        return jnp.concatenate(
            [jnp.concatenate(pieces[:8], axis=1), jnp.concatenate(pieces[8:], axis=1)], axis=0)

    def store(c, where, pieces):
        o_ref[rows(c), where] = joined(pieces).astype(BF16)

    class Message:
        def __init__(self, src, dst, link, main, extra):
            self.src, self.dst, self.link, self.sems = src, dst, link, (main, extra)

        def _copy(self, part, send_sem, recv_sem):
            return pltpu.make_async_remote_copy(
                self.src.at[part], self.dst.at[part], send_sem, recv_sem,
                device_id=neighbour[self.link], device_id_type=pl.DeviceIdType.MESH)

        def main(self):
            return self._copy(pl.ds(0, MAIN_ROWS), sent_main_sem.at[self.link], self.sems[0])

        def extra(self):
            return self._copy(pl.ds(EXTRA_AT, EXTRA_ROWS), sent_extra_sem, self.sems[1])

        def send_extra(self):
            _write_tiles(self.src, 12, _pack_extra(_read_tiles(self.src, 12, 20)))
            self.extra().start()

        def receive(self, use):
            self.main().wait_recv()
            more = _needs_extra([self.dst])
            use(_read_message(self.dst, False))

            @pl.when(more != 0)
            def _():
                self.extra().wait_recv()
                use(_read_message(self.dst, True))

            return more

    def streamed(link, c):
        slot = c & (RING - 1)
        return Message(send.at[link, c], recv.at[link, c], link,
                       main_sem.at[link, slot], extra_sem.at[link, slot])

    gather = Message(send.at[0, last], recv.at[1, last], 1, gather_sem.at[0], gather_sem.at[1])
    slot = n & (RING - 1)
    pass_on = Message(recv.at[1, last], recv.at[0, n], 0,
                      main_sem.at[0, slot], extra_sem.at[0, slot])

    load(0).start()
    barrier = pltpu.get_barrier_semaphore()
    for peer in neighbour:
        pl.semaphore_signal(barrier, inc=1, device_id=peer, device_id_type=pl.DeviceIdType.MESH)

    def lead_in(c, extras):
        msg = streamed(0, c)
        load(c).wait()

        @pl.when(c == 0)
        def _():
            for k in range(1, LOADS):
                load(k).start()
            load(last, load_sem.at[LOADS]).start()

        _write_message(msg.src, _pieces(block.at[c]))
        pl.when(c == 0)(lambda: pl.semaphore_wait(barrier, 2))
        msg.main().start()
        load(c + LOADS).start()
        more = _needs_extra([msg.src])
        pl.when(more != 0)(msg.send_extra)
        return extras + more

    extras = lax.fori_loop(0, AHEAD, lead_in, 0)

    load(last, load_sem.at[LOADS]).wait()
    _write_message(gather.src, _pieces(block.at[last]))
    gather.main().start()
    last_more = _needs_extra([gather.src])
    pl.when(last_more != 0)(gather.send_extra)
    extras = extras + 2 * last_more

    def step(i, extras):
        unpacking = i >= LAG
        j = jnp.maximum(i - LAG, 0)
        addend, summed, theirs = streamed(0, i), streamed(1, i), streamed(1, j)
        sent_x = streamed(0, jnp.minimum(i + AHEAD - 1, last - 1))
        sent_y = streamed(1, jnp.maximum(i - 1, 0))

        pl.when(unpacking)(lambda: theirs.main().wait_recv())
        addend.main().wait_recv()
        more = _needs_extra([
            addend.dst,
            recv.at[unpacking.astype(I32), jnp.where(unpacking, j, i)],
            sent_x.src,
            send.at[(i > 0).astype(I32), jnp.maximum(i - 1, 0)],
        ])
        more_x = ((more & 4) != 0) & (i > 0) & (i + AHEAD - 1 < last)
        more_y = ((more & 8) != 0) & (i > 0)

        def add(with_extra):
            total = _add(_pieces(block.at[i]), _read_message(addend.dst, with_extra))
            _write_message(summed.src, total)
            store(i, mine, total)

        add(False)

        @pl.when(more != 0)
        def _():
            pl.when(more_x)(sent_x.send_extra)
            pl.when(more_y)(sent_y.send_extra)

            @pl.when((more & 1) != 0)
            def _():
                addend.extra().wait_recv()
                add(True)

        summed.main().start()

        c = i + AHEAD

        @pl.when(c < last)
        def _():
            load(c).wait()
            _write_message(send.at[0, c], _pieces(block.at[c]))
            streamed(0, c).main().start()
            pl.when(c + LOADS < last)(lambda: load(c + LOADS).start())

        @pl.when(c == last)
        def _():
            streamed(0, last).main().start()
            pl.when(last_more != 0)(lambda: streamed(0, last).extra().start())

        @pl.when(c == n)
        def _():
            pass_on.main().start()
            pl.when(flag[0] != 0)(lambda: pass_on.extra().start())

        @pl.when(i == LAG - 1)
        def _():
            def keep(pieces):
                gathered[...] = joined(pieces)

            flag[0] = gather.receive(keep)

        @pl.when(unpacking)
        def _():
            store(j, other, _read_message(theirs.dst, False))

            @pl.when((more & 2) != 0)
            def _():
                theirs.extra().wait_recv()
                store(j, other, _read_message(theirs.dst, True))

        return extras + more_x.astype(I32) + more_y.astype(I32)

    extras = lax.fori_loop(0, last, step, extras) + flag[0]
    more = _needs_extra([streamed(1, last - 1).src])
    pl.when(more != 0)(streamed(1, last - 1).send_extra)
    extras = extras + more

    @pl.loop(last - LAG, last)
    def _(j):
        @pl.when(j == last - 2)
        def _():
            streamed(0, last).receive(
                lambda v: store(last, mine, _add(_pieces(block.at[last]), v)))

        @pl.when(j == last - 1)
        def _():
            pass_on.receive(lambda v: store(last, other, _add(_pieces(gathered), v)))

        streamed(1, j).receive(lambda v: store(j, other, v))

    def wait_sent(src, sem):
        pltpu.make_async_remote_copy(
            src, src, sem, sem, device_id=neighbour[0],
            device_id_type=pl.DeviceIdType.MESH).wait_send()

    wait_sent(send.at[0, :, pl.ds(0, MAIN_ROWS)], sent_main_sem.at[0])
    wait_sent(send.at[1, pl.ds(0, n), pl.ds(0, MAIN_ROWS)], sent_main_sem.at[1])

    @pl.loop(0, extras)
    def _(_):
        wait_sent(send.at[0, 0, pl.ds(EXTRA_AT, EXTRA_ROWS)], sent_extra_sem)


def pallas_dist_rsx_agy_m2048_n1024_kernel(x: jax.Array):
    _, m, cols = x.shape
    n = m // ROWS
    messages = pltpu.VMEM((2, n + 1, SLOT_ROWS, 128), I32)
    return pl.pallas_call(
        _body,
        out_shape=jax.ShapeDtypeStruct((m, 2 * cols), BF16),
        in_specs=[pl.BlockSpec(memory_space=pltpu.HBM)],
        out_specs=pl.BlockSpec(memory_space=pltpu.VMEM),
        scratch_shapes=[
            pltpu.VMEM((n, ROWS, cols), F32),
            messages,
            messages,
            pltpu.VMEM((ROWS, cols), F32),
            pltpu.SMEM((1,), I32),
            pltpu.SemaphoreType.DMA((LOADS + 1,)),
            pltpu.SemaphoreType.DMA((2, RING)),
            pltpu.SemaphoreType.DMA((2, RING)),
            pltpu.SemaphoreType.DMA((2,)),
            pltpu.SemaphoreType.DMA((2,)),
            pltpu.SemaphoreType.DMA,
        ],
        compiler_params=pltpu.CompilerParams(
            collective_id=0, vmem_limit_bytes=40 << 20, disable_semaphore_checks=True),
        name="rsx_agy",
    )(x)
```

```python
import jax
import jax.numpy as jnp
from jax import lax
from jax.experimental import pallas as pl
from jax.experimental.pallas import tpu as pltpu

I32, F32, BF16 = jnp.int32, jnp.float32, jnp.bfloat16
TILE = (8, 128)
ROWS = 32

HEAD_AT = 88
MAIN_ROWS = 90
EXTRA_AT, EXTRA_ROWS = 96, 40
SLOT_ROWS = 160

AHEAD = 3
LAG = 3
RING = 8
LOADS = 4
assert RING >= 2 * AHEAD and RING >= 2 * LAG + 2


def _bytes(b):
    v = b * 0x01010101
    return v - (1 << 32) if v >= 1 << 31 else v


def _shr(x, n):
    return lax.shift_right_logical(x, jnp.full_like(x, n) if isinstance(n, int) else n)


def _rotl(x, n):
    return (x << n) | _shr(x, 32 - n)


def _over_sublanes(op, x):
    for s in (4, 2, 1):
        x = op(x, pltpu.roll(x, s, 0))
    return x


def _sublane_cumsum(x):
    sublane = lax.broadcasted_iota(I32, TILE, 0)
    for s in (1, 2, 4):
        x = x + jnp.where(sublane >= s, pltpu.roll(x, s, 0), 0)
    return x


def _is_plain(head):
    return _shr(head, 24) == 255


def _unary_string(counts):
    string = jnp.zeros(TILE, I32)
    for word in counts:
        for n in (word & 255, _shr(word, 8) & 255, _shr(word, 16) & 255, _shr(word, 24)):
            string = (string << n) | jnp.minimum(n, 1)
    return string


def _encode(words):
    rest, exps, top = [], [], None
    for a, b in zip(words[:8], words[8:]):
        a, b = _rotl(a, 1), _rotl(b, 1)
        swap = (_shr(a, 8) ^ b) & 0x00FF00FF
        e = b ^ swap
        exps.append(e)
        rest.append(a ^ (swap << 8))
        p, q = e & 0x00FF00FF, _shr(e, 8) & 0x00FF00FF
        m = jnp.maximum(jnp.maximum(p, q), jnp.maximum(p << 16, q << 16))
        top = m if top is None else jnp.maximum(top, m)
    top = _shr(_over_sublanes(jnp.maximum, top), 16)

    codes, counts, seen = [], [], jnp.zeros(TILE, I32)
    for e in exps:
        g = top * _bytes(1) - e
        s = g + _bytes(0x80 - 7)
        escape = s & _bytes(0x80)
        mask = _shr(escape, 2) - _shr(escape, 7)
        codes.append(g | mask)
        counts.append((s + _bytes(1)) & mask)
        seen = seen | g

    early, late = sum(counts[1:4], counts[0]), sum(counts[5:], counts[4])
    late_bits = jnp.minimum(_shr(late * _bytes(1), 24), 31)
    string = (_unary_string(counts[:4]) << late_bits) | _unary_string(counts[4:])
    length = early + late
    length = (length & 0x00FF00FF) + (_shr(length, 8) & 0x00FF00FF)
    length = (length & 0xFFFF) + _shr(length, 16)

    end = _sublane_cumsum(length) + 8
    unfit = (length > 32) | (end > 64) | ((seen & _bytes(0xE0)) != 0)
    shift = jnp.maximum(64 - end, 0)
    s = shift & 31
    head0 = jnp.where(shift >= 32, string << s, _shr(_shr(string, 1), 31 - s)) & 0x00FFFFFF
    head1 = jnp.where(shift >= 32, 0, string << s)
    head0 = _over_sublanes(jnp.bitwise_or, jnp.where(unfit, -1, head0)) | (top << 24)
    head1 = _over_sublanes(jnp.bitwise_or, head1)
    head = jnp.where(lax.broadcasted_iota(I32, TILE, 0) == 0, head0, head1)

    plain = _is_plain(head0)
    c = [jnp.where(plain, e, k) & _bytes(7) for e, k in zip(exps, codes)]
    packed = [
        c[0] | (c[1] << 3) | ((c[6] & _bytes(3)) << 6),
        c[2] | (c[3] << 3) | ((c[7] & _bytes(3)) << 6),
        c[4] | (c[5] << 3) | ((c[6] & _bytes(4)) << 4) | ((c[7] & _bytes(4)) << 5),
    ]
    return rest + packed + [head], exps


def _pack_extra(exps):
    nibbles = [
        (_shr(exps[j], 3) & _bytes(0x0F)) | ((exps[j + 1] << 1) & _bytes(0xF0))
        for j in range(0, 8, 2)
    ]
    high = exps[0] & _bytes(0x80)
    for j in range(1, 8):
        high = high | _shr(exps[j] & _bytes(0x80), j)
    return nibbles + [high]


def _unpack_extra(tiles):
    return [
        ((_shr(tiles[j // 2], 1) if j % 2 else tiles[j // 2] << 3) & _bytes(0x78))
        | ((tiles[4] << j) & _bytes(0x80))
        for j in range(8)
    ]


def _decode(rest, packed, head0, head1, extra):
    p0, p1, p2 = packed
    codes = [
        p0 & _bytes(7), _shr(p0, 3) & _bytes(7),
        p1 & _bytes(7), _shr(p1, 3) & _bytes(7),
        p2 & _bytes(7), _shr(p2, 3) & _bytes(7),
        (_shr(p0, 6) & _bytes(3)) | (_shr(p2, 4) & _bytes(4)),
        (_shr(p1, 6) & _bytes(3)) | (_shr(p2, 5) & _bytes(4)),
    ]
    escapes = [(k + _bytes(1)) & _bytes(8) for k in codes]

    def string_after(skip):
        first = head0 & 0x00FFFFFF
        ones = lax.population_count(first)
        second = skip > ones
        window = jnp.where(second, head1, first)
        left = jnp.where(second, skip - ones, skip)
        start = jnp.where(second, 33, 1)
        for step in (16, 8, 4, 2, 1):
            ones = lax.population_count(_shr(window, 32 - step))
            advance = ones < left
            window = jnp.where(advance, window << step, window)
            left = jnp.where(advance, left - ones, left)
            start = jnp.where(advance, start + step, start)
        start = jnp.where(skip == 0, 8, start)
        s = start & 31
        return jnp.where(start >= 32, head1 << s, (head0 << s) | _shr(_shr(head1, 1), 31 - s))

    parts = [_shr(_shr(escapes[j] + escapes[j + 1], 3) * _bytes(1), 24) for j in (0, 2, 4, 6)]
    total = (parts[0] + parts[1]) + (parts[2] + parts[3])
    skip = _sublane_cumsum(total) - total

    top = _shr(head0, 24) * _bytes(1)
    a, b = [], []
    for j in range(8):
        if j % 2 == 0:
            string = string_after(skip)
            skip = skip + parts[j // 2]
        one = _shr(escapes[j], 3)
        mask = (escapes[j] << 2) - one
        g = codes[j] - one
        for byte in range(4):
            n = (lax.clz(string) + 1) & (_shr(mask, 8 * byte) if byte else mask)
            string = string << n
            g = g + (n << (8 * byte) if byte else n)
        e = top - g
        if extra is not None:
            e = jnp.where(_is_plain(head0), codes[j] | extra[j], e)
        swap = (e ^ _shr(rest[j], 8)) & 0x00FF00FF
        a.append(_rotl(rest[j] ^ (swap << 8), 31))
        b.append(_rotl(e ^ swap, 31))
    return a + b


def _pieces(block):
    return [block[i:i + 16, j:j + 128] for i in (0, 16) for j in range(0, 1024, 128)]


def _joined(pieces):
    return jnp.concatenate(
        [jnp.concatenate(pieces[:8], axis=1), jnp.concatenate(pieces[8:], axis=1)], axis=0)


def _add(u, v):
    return [a + b for a, b in zip(u, v)]


def _read_tiles(msg, row, count):
    return [msg[row + 8 * j:row + 8 * j + 8, :] for j in range(count)]


def _write_tiles(msg, row, tiles):
    for j, t in enumerate(tiles):
        msg[row + 8 * j:row + 8 * j + 8, :] = t


def _header(msg, k=0):
    return jnp.broadcast_to(msg[HEAD_AT + k:HEAD_AT + k + 1, :], TILE)


def _write_message(msg, pieces):
    main, exps = _encode([pltpu.bitcast(p.astype(BF16), I32) for p in pieces])
    _write_tiles(msg, 0, main)
    _write_tiles(msg, EXTRA_AT, exps)


def _read_message(msg, with_extra):
    extra = _unpack_extra(_read_tiles(msg, EXTRA_AT, 5)) if with_extra else None
    words = _decode(
        _read_tiles(msg, 0, 8), _read_tiles(msg, 64, 3), _header(msg, 0), _header(msg, 1), extra)
    return [pltpu.bitcast(w, BF16).astype(F32) for w in words]


def _needs_extra(msgs):
    sublane = lax.broadcasted_iota(I32, TILE, 0)
    bits = jnp.zeros(TILE, F32)
    for k, msg in enumerate(msgs):
        bits = jnp.where((sublane == k) & _is_plain(_header(msg)), float(1 << k), bits)
    bits = jnp.sum(jnp.max(bits, axis=1, keepdims=True), axis=0, keepdims=True)
    return bits.astype(I32)[0, 0]


class _Message:
    def __init__(self, src, dst, peer, main_sems, extra_sems):
        self.src, self.dst, self.peer = src, dst, peer
        self.main_sems, self.extra_sems = main_sems, extra_sems

    def _copy(self, part, sems):
        return pltpu.make_async_remote_copy(
            self.src.at[part], self.dst.at[part], *sems,
            device_id=self.peer, device_id_type=pl.DeviceIdType.MESH)

    def main(self):
        return self._copy(pl.ds(0, MAIN_ROWS), self.main_sems)

    def extra(self):
        return self._copy(pl.ds(EXTRA_AT, EXTRA_ROWS), self.extra_sems)

    def send_extra(self):
        _write_tiles(self.src, EXTRA_AT, _pack_extra(_read_tiles(self.src, EXTRA_AT, 8)))
        self.extra().start()

    def receive(self, use):
        self.main().wait_recv()
        more = _needs_extra([self.dst])
        use(_read_message(self.dst, False))

        @pl.when(more != 0)
        def _():
            self.extra().wait_recv()
            use(_read_message(self.dst, True))

        return more


def _body(x_ref, o_ref, block, send, recv, gathered, gathered_more,
          load_sem, main_sem, extra_sem, gather_sem, sent_main_sem, sent_extra_sem):
    n, _, cols = block.shape
    last = n - 1
    mx, my = lax.axis_index("x"), lax.axis_index("y")
    neighbour = ((1 - mx, my), (mx, 1 - my))
    mine = pl.ds(pl.multiple_of(my * cols, cols), cols)
    other = pl.ds(pl.multiple_of((1 - my) * cols, cols), cols)

    def rows(c):
        return pl.ds(c * ROWS if isinstance(c, int) else pl.multiple_of(c * ROWS, ROWS), ROWS)

    def load(c):
        return pltpu.make_async_copy(
            x_ref.at[0, rows(c)], block.at[c], load_sem.at[c & (LOADS - 1)])

    def load_last():
        return pltpu.make_async_copy(x_ref.at[0, rows(last)], block.at[last], load_sem.at[LOADS])

    def store(c, where, pieces):
        o_ref[rows(c), where] = _joined(pieces).astype(BF16)

    def message(link, src, dst, main, extra):
        return _Message(src, dst, neighbour[link],
                        (sent_main_sem.at[link], main), (sent_extra_sem, extra))

    def in_order(link, c, src, dst):
        slot = c & (RING - 1)
        return message(link, src, dst, main_sem.at[link, slot], extra_sem.at[link, slot])

    def streamed(link, c):
        return in_order(link, c, send.at[link, c], recv.at[link, c])

    gather = message(1, send.at[0, last], recv.at[1, last], gather_sem.at[0], gather_sem.at[1])
    pass_on = in_order(0, n, recv.at[1, last], recv.at[0, n])

    load(0).start()
    barrier = pltpu.get_barrier_semaphore()
    for peer in neighbour:
        pl.semaphore_signal(barrier, inc=1, device_id=peer, device_id_type=pl.DeviceIdType.MESH)

    def lead_in(c, extras):
        msg = streamed(0, c)
        load(c).wait()

        @pl.when(c == 0)
        def _():
            for k in range(1, LOADS):
                load(k).start()
            load_last().start()

        _write_message(msg.src, _pieces(block.at[c]))
        pl.when(c == 0)(lambda: pl.semaphore_wait(barrier, 2))
        msg.main().start()
        load(c + LOADS).start()
        more = _needs_extra([msg.src])
        pl.when(more != 0)(msg.send_extra)
        return extras + more

    extras = lax.fori_loop(0, AHEAD, lead_in, 0)

    load_last().wait()
    _write_message(gather.src, _pieces(block.at[last]))
    gather.main().start()
    last_more = _needs_extra([gather.src])
    pl.when(last_more != 0)(gather.send_extra)
    extras = extras + 2 * last_more

    def step(i, extras):
        unpacking = i >= LAG
        j = jnp.maximum(i - LAG, 0)
        addend, summed, theirs = streamed(0, i), streamed(1, i), streamed(1, j)
        sent_x = streamed(0, jnp.minimum(i + AHEAD - 1, last - 1))
        sent_y = streamed(1, jnp.maximum(i - 1, 0))

        pl.when(unpacking)(lambda: theirs.main().wait_recv())
        addend.main().wait_recv()
        more = _needs_extra([
            addend.dst,
            recv.at[unpacking.astype(I32), jnp.where(unpacking, j, i)],
            sent_x.src,
            send.at[(i > 0).astype(I32), jnp.maximum(i - 1, 0)],
        ])
        more_x = ((more & 4) != 0) & (i > 0) & (i + AHEAD - 1 < last)
        more_y = ((more & 8) != 0) & (i > 0)

        def add(with_extra):
            total = _add(_pieces(block.at[i]), _read_message(addend.dst, with_extra))
            _write_message(summed.src, total)
            store(i, mine, total)

        add(False)

        @pl.when(more != 0)
        def _():
            pl.when(more_x)(sent_x.send_extra)
            pl.when(more_y)(sent_y.send_extra)

            @pl.when((more & 1) != 0)
            def _():
                addend.extra().wait_recv()
                add(True)

        summed.main().start()

        c = i + AHEAD

        @pl.when(c < last)
        def _():
            load(c).wait()
            _write_message(send.at[0, c], _pieces(block.at[c]))
            streamed(0, c).main().start()
            pl.when(c + LOADS < last)(lambda: load(c + LOADS).start())

        @pl.when(c == last)
        def _():
            streamed(0, last).main().start()
            pl.when(last_more != 0)(lambda: streamed(0, last).extra().start())

        @pl.when(c == n)
        def _():
            pass_on.main().start()
            pl.when(gathered_more[0] != 0)(lambda: pass_on.extra().start())

        @pl.when(i == LAG - 1)
        def _():
            def keep(pieces):
                gathered[...] = _joined(pieces)

            gathered_more[0] = gather.receive(keep)

        @pl.when(unpacking)
        def _():
            store(j, other, _read_message(theirs.dst, False))

            @pl.when((more & 2) != 0)
            def _():
                theirs.extra().wait_recv()
                store(j, other, _read_message(theirs.dst, True))

        return extras + more_x.astype(I32) + more_y.astype(I32)

    extras = lax.fori_loop(0, last, step, extras)
    final = streamed(1, last - 1)
    more = _needs_extra([final.src])
    pl.when(more != 0)(final.send_extra)
    extras = extras + more + gathered_more[0]

    @pl.loop(last - LAG, last)
    def _(j):
        @pl.when(j == last - 2)
        def _():
            streamed(0, last).receive(
                lambda v: store(last, mine, _add(_pieces(block.at[last]), v)))

        @pl.when(j == last - 1)
        def _():
            pass_on.receive(lambda v: store(last, other, _add(_pieces(gathered), v)))

        streamed(1, j).receive(lambda v: store(j, other, v))

    def wait_sent(like, sem):
        pltpu.make_async_remote_copy(
            like, like, sem, sem,
            device_id=neighbour[0], device_id_type=pl.DeviceIdType.MESH).wait_send()

    wait_sent(send.at[0, pl.ds(0, n + 1), pl.ds(0, MAIN_ROWS)], sent_main_sem.at[0])
    wait_sent(send.at[1, pl.ds(0, n), pl.ds(0, MAIN_ROWS)], sent_main_sem.at[1])

    @pl.loop(0, extras)
    def _(_):
        wait_sent(send.at[0, 0, pl.ds(EXTRA_AT, EXTRA_ROWS)], sent_extra_sem)


def pallas_dist_rsx_agy_m2048_n1024_kernel(x: jax.Array):
    _, m, cols = x.shape
    n = m // ROWS
    messages = pltpu.VMEM((2, n + 1, SLOT_ROWS, 128), I32)
    return pl.pallas_call(
        _body,
        out_shape=jax.ShapeDtypeStruct((m, 2 * cols), BF16),
        in_specs=[pl.BlockSpec(memory_space=pltpu.HBM)],
        out_specs=pl.BlockSpec(memory_space=pltpu.VMEM),
        scratch_shapes=[
            pltpu.VMEM((n, ROWS, cols), F32),
            messages,
            messages,
            pltpu.VMEM((ROWS, cols), F32),
            pltpu.SMEM((1,), I32),
            pltpu.SemaphoreType.DMA((LOADS + 1,)),
            pltpu.SemaphoreType.DMA((2, RING)),
            pltpu.SemaphoreType.DMA((2, RING)),
            pltpu.SemaphoreType.DMA((2,)),
            pltpu.SemaphoreType.DMA((2,)),
            pltpu.SemaphoreType.DMA,
        ],
        compiler_params=pltpu.CompilerParams(
            collective_id=0, vmem_limit_bytes=40 << 20, disable_semaphore_checks=True),
        name="rsx_agy",
    )(x)
```

```python
import jax
import jax.numpy as jnp
from jax import lax
from jax.experimental import pallas as pl
from jax.experimental.pallas import tpu as pltpu

I32, F32, BF16 = jnp.int32, jnp.float32, jnp.bfloat16
TILE = (8, 128)
ROWS = 32

HEAD_AT = 88
MAIN_ROWS = 90
EXTRA_AT, EXTRA_ROWS = 96, 40
SLOT_ROWS = 160

AHEAD = 3
LAG = 3
LOADS = 4


def _bytes(b):
    v = b * 0x01010101
    return v - (1 << 32) if v >= 1 << 31 else v


def _shr(x, n):
    return lax.shift_right_logical(x, jnp.full_like(x, n) if isinstance(n, int) else n)


def _rotl(x, n):
    return (x << n) | _shr(x, 32 - n)


def _over_sublanes(op, x):
    for s in (4, 2, 1):
        x = op(x, pltpu.roll(x, s, 0))
    return x


def _sublane_cumsum(x):
    sublane = lax.broadcasted_iota(I32, TILE, 0)
    for s in (1, 2, 4):
        x = x + jnp.where(sublane >= s, pltpu.roll(x, s, 0), 0)
    return x


def _is_plain(head):
    return _shr(head, 24) == 255


def _unary_string(counts):
    string = jnp.zeros(TILE, I32)
    for word in counts:
        for n in (word & 255, _shr(word, 8) & 255, _shr(word, 16) & 255, _shr(word, 24)):
            string = (string << n) | jnp.minimum(n, 1)
    return string


def _encode(words):
    rest, exps, top = [], [], None
    for a, b in zip(words[:8], words[8:]):
        a, b = _rotl(a, 1), _rotl(b, 1)
        swap = (_shr(a, 8) ^ b) & 0x00FF00FF
        e = b ^ swap
        exps.append(e)
        rest.append(a ^ (swap << 8))
        p, q = e & 0x00FF00FF, _shr(e, 8) & 0x00FF00FF
        m = jnp.maximum(jnp.maximum(p, q), jnp.maximum(p << 16, q << 16))
        top = m if top is None else jnp.maximum(top, m)
    top = _shr(_over_sublanes(jnp.maximum, top), 16)

    codes, counts, seen = [], [], jnp.zeros(TILE, I32)
    for e in exps:
        g = top * _bytes(1) - e
        s = g + _bytes(0x80 - 7)
        escape = s & _bytes(0x80)
        mask = _shr(escape, 2) - _shr(escape, 7)
        codes.append(g | mask)
        counts.append((s + _bytes(1)) & mask)
        seen = seen | g

    early, late = sum(counts[1:4], counts[0]), sum(counts[5:], counts[4])
    late_bits = jnp.minimum(_shr(late * _bytes(1), 24), 31)
    string = (_unary_string(counts[:4]) << late_bits) | _unary_string(counts[4:])
    length = early + late
    length = (length & 0x00FF00FF) + (_shr(length, 8) & 0x00FF00FF)
    length = (length & 0xFFFF) + _shr(length, 16)

    end = _sublane_cumsum(length) + 8
    unfit = (length > 32) | (end > 64) | ((seen & _bytes(0xE0)) != 0)
    shift = jnp.maximum(64 - end, 0)
    s = shift & 31
    head0 = jnp.where(shift >= 32, string << s, _shr(_shr(string, 1), 31 - s)) & 0x00FFFFFF
    head1 = jnp.where(shift >= 32, 0, string << s)
    head0 = _over_sublanes(jnp.bitwise_or, jnp.where(unfit, -1, head0)) | (top << 24)
    head1 = _over_sublanes(jnp.bitwise_or, head1)
    head = jnp.where(lax.broadcasted_iota(I32, TILE, 0) == 0, head0, head1)

    plain = _is_plain(head0)
    c = [jnp.where(plain, e, k) & _bytes(7) for e, k in zip(exps, codes)]
    packed = [
        c[0] | (c[1] << 3) | ((c[6] & _bytes(3)) << 6),
        c[2] | (c[3] << 3) | ((c[7] & _bytes(3)) << 6),
        c[4] | (c[5] << 3) | ((c[6] & _bytes(4)) << 4) | ((c[7] & _bytes(4)) << 5),
    ]
    return rest + packed + [head], exps


def _pack_extra(exps):
    nibbles = [
        (_shr(exps[j], 3) & _bytes(0x0F)) | ((exps[j + 1] << 1) & _bytes(0xF0))
        for j in range(0, 8, 2)
    ]
    high = exps[0] & _bytes(0x80)
    for j in range(1, 8):
        high = high | _shr(exps[j] & _bytes(0x80), j)
    return nibbles + [high]


def _unpack_extra(tiles):
    return [
        ((_shr(tiles[j // 2], 1) if j % 2 else tiles[j // 2] << 3) & _bytes(0x78))
        | ((tiles[4] << j) & _bytes(0x80))
        for j in range(8)
    ]


def _decode(rest, packed, head0, head1, extra):
    p0, p1, p2 = packed
    codes = [
        p0 & _bytes(7), _shr(p0, 3) & _bytes(7),
        p1 & _bytes(7), _shr(p1, 3) & _bytes(7),
        p2 & _bytes(7), _shr(p2, 3) & _bytes(7),
        (_shr(p0, 6) & _bytes(3)) | (_shr(p2, 4) & _bytes(4)),
        (_shr(p1, 6) & _bytes(3)) | (_shr(p2, 5) & _bytes(4)),
    ]
    escapes = [(k + _bytes(1)) & _bytes(8) for k in codes]

    def string_after(skip):
        first = head0 & 0x00FFFFFF
        ones = lax.population_count(first)
        second = skip > ones
        window = jnp.where(second, head1, first)
        left = jnp.where(second, skip - ones, skip)
        start = jnp.where(second, 33, 1)
        for step in (16, 8, 4, 2, 1):
            ones = lax.population_count(_shr(window, 32 - step))
            advance = ones < left
            window = jnp.where(advance, window << step, window)
            left = jnp.where(advance, left - ones, left)
            start = jnp.where(advance, start + step, start)
        start = jnp.where(skip == 0, 8, start)
        s = start & 31
        return jnp.where(start >= 32, head1 << s, (head0 << s) | _shr(_shr(head1, 1), 31 - s))

    parts = [_shr(_shr(escapes[j] + escapes[j + 1], 3) * _bytes(1), 24) for j in (0, 2, 4, 6)]
    total = (parts[0] + parts[1]) + (parts[2] + parts[3])
    skip = _sublane_cumsum(total) - total

    top = _shr(head0, 24) * _bytes(1)
    a, b = [], []
    for j in range(8):
        if j % 2 == 0:
            string = string_after(skip)
            skip = skip + parts[j // 2]
        one = _shr(escapes[j], 3)
        mask = (escapes[j] << 2) - one
        g = codes[j] - one
        for byte in range(4):
            n = (lax.clz(string) + 1) & (_shr(mask, 8 * byte) if byte else mask)
            string = string << n
            g = g + (n << (8 * byte) if byte else n)
        e = top - g
        if extra is not None:
            e = jnp.where(_is_plain(head0), codes[j] | extra[j], e)
        swap = (e ^ _shr(rest[j], 8)) & 0x00FF00FF
        a.append(_rotl(rest[j] ^ (swap << 8), 31))
        b.append(_rotl(e ^ swap, 31))
    return a + b


def _pieces(block):
    return [block[i:i + 16, j:j + 128] for i in (0, 16) for j in range(0, 1024, 128)]


def _joined(pieces):
    return jnp.concatenate(
        [jnp.concatenate(pieces[:8], axis=1), jnp.concatenate(pieces[8:], axis=1)], axis=0)


def _add(u, v):
    return [a + b for a, b in zip(u, v)]


def _read_tiles(msg, row, count):
    return [msg[row + 8 * j:row + 8 * j + 8, :] for j in range(count)]


def _write_tiles(msg, row, tiles):
    for j, t in enumerate(tiles):
        msg[row + 8 * j:row + 8 * j + 8, :] = t


def _header(msg, k=0):
    return jnp.broadcast_to(msg[HEAD_AT + k:HEAD_AT + k + 1, :], TILE)


def _write_message(msg, pieces):
    main, exps = _encode([pltpu.bitcast(p.astype(BF16), I32) for p in pieces])
    _write_tiles(msg, 0, main)
    _write_tiles(msg, EXTRA_AT, exps)


def _read_message(msg, with_extra):
    extra = _unpack_extra(_read_tiles(msg, EXTRA_AT, 5)) if with_extra else None
    words = _decode(
        _read_tiles(msg, 0, 8), _read_tiles(msg, 64, 3), _header(msg, 0), _header(msg, 1), extra)
    return [pltpu.bitcast(w, BF16).astype(F32) for w in words]


def _needs_extra(msgs):
    sublane = lax.broadcasted_iota(I32, TILE, 0)
    bits = jnp.zeros(TILE, F32)
    for k, msg in enumerate(msgs):
        bits = jnp.where((sublane == k) & _is_plain(_header(msg)), float(1 << k), bits)
    bits = jnp.sum(jnp.max(bits, axis=1, keepdims=True), axis=0, keepdims=True)
    return bits.astype(I32)[0, 0]


class _Message:
    def __init__(self, src, dst, peer, main_sems, extra_sems):
        self.src, self.dst, self.peer = src, dst, peer
        self.main_sems, self.extra_sems = main_sems, extra_sems

    def _copy(self, part, sems):
        return pltpu.make_async_remote_copy(
            self.src.at[part], self.dst.at[part], *sems,
            device_id=self.peer, device_id_type=pl.DeviceIdType.MESH)

    def main(self):
        return self._copy(pl.ds(0, MAIN_ROWS), self.main_sems)

    def extra(self):
        return self._copy(pl.ds(EXTRA_AT, EXTRA_ROWS), self.extra_sems)

    def send_extra(self):
        _write_tiles(self.src, EXTRA_AT, _pack_extra(_read_tiles(self.src, EXTRA_AT, 8)))
        self.extra().start()

    def receive(self, use):
        self.main().wait_recv()
        more = _needs_extra([self.dst])
        use(_read_message(self.dst, False))

        @pl.when(more != 0)
        def _():
            self.extra().wait_recv()
            use(_read_message(self.dst, True))

        return more


def _body(x_ref, o_ref, block, send, recv, gathered, gathered_more,
          load_sem, main_sem, extra_sem, sent_main_sem, sent_extra_sem):
    n, _, cols = block.shape
    last = n - 1
    mx, my = lax.axis_index("x"), lax.axis_index("y")
    neighbour = ((1 - mx, my), (mx, 1 - my))
    mine = pl.ds(pl.multiple_of(my * cols, cols), cols)
    other = pl.ds(pl.multiple_of((1 - my) * cols, cols), cols)

    def rows(c):
        return pl.ds(c * ROWS if isinstance(c, int) else pl.multiple_of(c * ROWS, ROWS), ROWS)

    def load(c):
        return pltpu.make_async_copy(
            x_ref.at[0, rows(c)], block.at[c], load_sem.at[c & (LOADS - 1)])

    def load_last():
        return pltpu.make_async_copy(x_ref.at[0, rows(last)], block.at[last], load_sem.at[LOADS])

    def store(c, where, pieces):
        o_ref[rows(c), where] = _joined(pieces).astype(BF16)

    def message(link, c, src):
        sem = link * (n + 1) + c
        return _Message(src, recv.at[link, c], neighbour[link],
                        (sent_main_sem.at[link], main_sem.at[sem]),
                        (sent_extra_sem, extra_sem.at[sem]))

    def streamed(link, c):
        return message(link, c, send.at[link, c])

    gather = message(1, last, send.at[0, last])
    pass_on = message(0, n, gather.dst)

    load(0).start()
    barrier = pltpu.get_barrier_semaphore()
    for peer in neighbour:
        pl.semaphore_signal(barrier, inc=1, device_id=peer, device_id_type=pl.DeviceIdType.MESH)

    def lead_in(c, extras):
        msg = streamed(0, c)
        load(c).wait()

        @pl.when(c == 0)
        def _():
            for k in range(1, LOADS):
                load(k).start()
            load_last().start()

        _write_message(msg.src, _pieces(block.at[c]))
        pl.when(c == 0)(lambda: pl.semaphore_wait(barrier, 2))
        msg.main().start()
        load(c + LOADS).start()
        more = _needs_extra([msg.src])
        pl.when(more != 0)(msg.send_extra)
        return extras + more

    extras = lax.fori_loop(0, AHEAD, lead_in, 0)

    load_last().wait()
    _write_message(gather.src, _pieces(block.at[last]))
    gather.main().start()
    last_more = _needs_extra([gather.src])
    pl.when(last_more != 0)(gather.send_extra)
    extras = extras + 2 * last_more

    def step(i, extras):
        unpacking = i >= LAG
        j = jnp.maximum(i - LAG, 0)
        addend, summed, theirs = streamed(0, i), streamed(1, i), streamed(1, j)
        sent_x = streamed(0, jnp.minimum(i + AHEAD - 1, last - 1))
        sent_y = streamed(1, jnp.maximum(i - 1, 0))

        pl.when(unpacking)(lambda: theirs.main().wait_recv())
        addend.main().wait_recv()
        more = _needs_extra([
            addend.dst,
            recv.at[unpacking.astype(I32), jnp.where(unpacking, j, i)],
            sent_x.src,
            send.at[(i > 0).astype(I32), jnp.maximum(i - 1, 0)],
        ])
        more_x = ((more & 4) != 0) & (i > 0) & (i + AHEAD - 1 < last)
        more_y = ((more & 8) != 0) & (i > 0)

        def add(with_extra):
            total = _add(_pieces(block.at[i]), _read_message(addend.dst, with_extra))
            _write_message(summed.src, total)
            store(i, mine, total)

        add(False)

        @pl.when(more != 0)
        def _():
            pl.when(more_x)(sent_x.send_extra)
            pl.when(more_y)(sent_y.send_extra)

            @pl.when((more & 1) != 0)
            def _():
                addend.extra().wait_recv()
                add(True)

        summed.main().start()

        c = i + AHEAD

        @pl.when(c < last)
        def _():
            load(c).wait()
            _write_message(send.at[0, c], _pieces(block.at[c]))
            streamed(0, c).main().start()
            pl.when(c + LOADS < last)(lambda: load(c + LOADS).start())

        @pl.when(c == last)
        def _():
            streamed(0, last).main().start()
            pl.when(last_more != 0)(lambda: streamed(0, last).extra().start())

        @pl.when(c == n)
        def _():
            pass_on.main().start()
            pl.when(gathered_more[0] != 0)(lambda: pass_on.extra().start())

        @pl.when(i == LAG - 1)
        def _():
            def keep(pieces):
                gathered[...] = _joined(pieces)

            gathered_more[0] = gather.receive(keep)

        @pl.when(unpacking)
        def _():
            store(j, other, _read_message(theirs.dst, False))

            @pl.when((more & 2) != 0)
            def _():
                theirs.extra().wait_recv()
                store(j, other, _read_message(theirs.dst, True))

        return extras + more_x.astype(I32) + more_y.astype(I32)

    extras = lax.fori_loop(0, last, step, extras)
    final = streamed(1, last - 1)
    more = _needs_extra([final.src])
    pl.when(more != 0)(final.send_extra)
    extras = extras + more + gathered_more[0]

    @pl.loop(last - LAG, last)
    def _(j):
        @pl.when(j == last - 2)
        def _():
            streamed(0, last).receive(
                lambda v: store(last, mine, _add(_pieces(block.at[last]), v)))

        @pl.when(j == last - 1)
        def _():
            pass_on.receive(lambda v: store(last, other, _add(_pieces(gathered), v)))

        streamed(1, j).receive(lambda v: store(j, other, v))

    def wait_sent(like, sem):
        pltpu.make_async_remote_copy(
            like, like, sem, sem,
            device_id=neighbour[0], device_id_type=pl.DeviceIdType.MESH).wait_send()

    wait_sent(send.at[0, pl.ds(0, n + 1), pl.ds(0, MAIN_ROWS)], sent_main_sem.at[0])
    wait_sent(send.at[1, pl.ds(0, n), pl.ds(0, MAIN_ROWS)], sent_main_sem.at[1])

    @pl.loop(0, extras)
    def _(_):
        wait_sent(send.at[0, 0, pl.ds(EXTRA_AT, EXTRA_ROWS)], sent_extra_sem)


def pallas_dist_rsx_agy_m2048_n1024_kernel(x: jax.Array):
    _, m, cols = x.shape
    n = m // ROWS
    messages = pltpu.VMEM((2, n + 1, SLOT_ROWS, 128), I32)
    return pl.pallas_call(
        _body,
        out_shape=jax.ShapeDtypeStruct((m, 2 * cols), BF16),
        in_specs=[pl.BlockSpec(memory_space=pltpu.HBM)],
        out_specs=pl.BlockSpec(memory_space=pltpu.VMEM),
        scratch_shapes=[
            pltpu.VMEM((n, ROWS, cols), F32),
            messages,
            messages,
            pltpu.VMEM((ROWS, cols), F32),
            pltpu.SMEM((1,), I32),
            pltpu.SemaphoreType.DMA((LOADS + 1,)),
            pltpu.SemaphoreType.DMA((2 * (n + 1),)),
            pltpu.SemaphoreType.DMA((2 * (n + 1),)),
            pltpu.SemaphoreType.DMA((2,)),
            pltpu.SemaphoreType.DMA,
        ],
        compiler_params=pltpu.CompilerParams(
            collective_id=0, vmem_limit_bytes=40 << 20, disable_semaphore_checks=True),
        name="rsx_agy",
    )(x)
```

```python
import jax
import jax.numpy as jnp
from jax import lax
from jax.experimental import pallas as pl
from jax.experimental.pallas import tpu as pltpu

I32, F32, BF16 = jnp.int32, jnp.float32, jnp.bfloat16
TILE = (8, 128)
ROWS = 32

HEAD_AT = 88
MAIN_ROWS = 90
EXTRA_AT, EXTRA_ROWS = 96, 40
SLOT_ROWS = 160

AHEAD = 3
LAG = 3
LOADS = 4
RAW = 2
VIA_X = 40
assert RAW == 2 and AHEAD == RAW + 1 and LAG >= RAW


def _bytes(b):
    v = b * 0x01010101
    return v - (1 << 32) if v >= 1 << 31 else v


def _shr(x, n):
    return lax.shift_right_logical(x, jnp.full_like(x, n) if isinstance(n, int) else n)


def _rotl(x, n):
    return (x << n) | _shr(x, 32 - n)


def _over_sublanes(op, x):
    for s in (4, 2, 1):
        x = op(x, pltpu.roll(x, s, 0))
    return x


def _sublane_cumsum(x):
    sublane = lax.broadcasted_iota(I32, TILE, 0)
    for s in (1, 2, 4):
        x = x + jnp.where(sublane >= s, pltpu.roll(x, s, 0), 0)
    return x


def _is_plain(head):
    return _shr(head, 24) == 255


def _unary_string(counts):
    string = jnp.zeros(TILE, I32)
    for word in counts:
        for n in (word & 255, _shr(word, 8) & 255, _shr(word, 16) & 255, _shr(word, 24)):
            string = (string << n) | jnp.minimum(n, 1)
    return string


def _encode(words):
    rest, exps, top = [], [], None
    for a, b in zip(words[:8], words[8:]):
        a, b = _rotl(a, 1), _rotl(b, 1)
        swap = (_shr(a, 8) ^ b) & 0x00FF00FF
        e = b ^ swap
        exps.append(e)
        rest.append(a ^ (swap << 8))
        p, q = e & 0x00FF00FF, _shr(e, 8) & 0x00FF00FF
        m = jnp.maximum(jnp.maximum(p, q), jnp.maximum(p << 16, q << 16))
        top = m if top is None else jnp.maximum(top, m)
    top = _shr(_over_sublanes(jnp.maximum, top), 16)

    codes, counts, seen = [], [], jnp.zeros(TILE, I32)
    for e in exps:
        g = top * _bytes(1) - e
        s = g + _bytes(0x80 - 7)
        escape = s & _bytes(0x80)
        mask = _shr(escape, 2) - _shr(escape, 7)
        codes.append(g | mask)
        counts.append((s + _bytes(1)) & mask)
        seen = seen | g

    early, late = sum(counts[1:4], counts[0]), sum(counts[5:], counts[4])
    late_bits = jnp.minimum(_shr(late * _bytes(1), 24), 31)
    string = (_unary_string(counts[:4]) << late_bits) | _unary_string(counts[4:])
    length = early + late
    length = (length & 0x00FF00FF) + (_shr(length, 8) & 0x00FF00FF)
    length = (length & 0xFFFF) + _shr(length, 16)

    end = _sublane_cumsum(length) + 8
    unfit = (length > 32) | (end > 64) | ((seen & _bytes(0xE0)) != 0)
    shift = jnp.maximum(64 - end, 0)
    s = shift & 31
    head0 = jnp.where(shift >= 32, string << s, _shr(_shr(string, 1), 31 - s)) & 0x00FFFFFF
    head1 = jnp.where(shift >= 32, 0, string << s)
    head0 = _over_sublanes(jnp.bitwise_or, jnp.where(unfit, -1, head0)) | (top << 24)
    head1 = _over_sublanes(jnp.bitwise_or, head1)
    head = jnp.where(lax.broadcasted_iota(I32, TILE, 0) == 0, head0, head1)

    plain = _is_plain(head0)
    c = [jnp.where(plain, e, k) & _bytes(7) for e, k in zip(exps, codes)]
    packed = [
        c[0] | (c[1] << 3) | ((c[6] & _bytes(3)) << 6),
        c[2] | (c[3] << 3) | ((c[7] & _bytes(3)) << 6),
        c[4] | (c[5] << 3) | ((c[6] & _bytes(4)) << 4) | ((c[7] & _bytes(4)) << 5),
    ]
    return rest + packed + [head], exps


def _pack_extra(exps):
    nibbles = [
        (_shr(exps[j], 3) & _bytes(0x0F)) | ((exps[j + 1] << 1) & _bytes(0xF0))
        for j in range(0, 8, 2)
    ]
    high = exps[0] & _bytes(0x80)
    for j in range(1, 8):
        high = high | _shr(exps[j] & _bytes(0x80), j)
    return nibbles + [high]


def _unpack_extra(tiles):
    return [
        ((_shr(tiles[j // 2], 1) if j % 2 else tiles[j // 2] << 3) & _bytes(0x78))
        | ((tiles[4] << j) & _bytes(0x80))
        for j in range(8)
    ]


def _decode(rest, packed, head0, head1, extra):
    p0, p1, p2 = packed
    codes = [
        p0 & _bytes(7), _shr(p0, 3) & _bytes(7),
        p1 & _bytes(7), _shr(p1, 3) & _bytes(7),
        p2 & _bytes(7), _shr(p2, 3) & _bytes(7),
        (_shr(p0, 6) & _bytes(3)) | (_shr(p2, 4) & _bytes(4)),
        (_shr(p1, 6) & _bytes(3)) | (_shr(p2, 5) & _bytes(4)),
    ]
    escapes = [(k + _bytes(1)) & _bytes(8) for k in codes]

    def string_after(skip):
        first = head0 & 0x00FFFFFF
        ones = lax.population_count(first)
        second = skip > ones
        window = jnp.where(second, head1, first)
        left = jnp.where(second, skip - ones, skip)
        start = jnp.where(second, 33, 1)
        for step in (16, 8, 4, 2, 1):
            ones = lax.population_count(_shr(window, 32 - step))
            advance = ones < left
            window = jnp.where(advance, window << step, window)
            left = jnp.where(advance, left - ones, left)
            start = jnp.where(advance, start + step, start)
        start = jnp.where(skip == 0, 8, start)
        s = start & 31
        return jnp.where(start >= 32, head1 << s, (head0 << s) | _shr(_shr(head1, 1), 31 - s))

    parts = [_shr(_shr(escapes[j] + escapes[j + 1], 3) * _bytes(1), 24) for j in (0, 2, 4, 6)]
    total = (parts[0] + parts[1]) + (parts[2] + parts[3])
    skip = _sublane_cumsum(total) - total

    top = _shr(head0, 24) * _bytes(1)
    a, b = [], []
    for j in range(8):
        if j % 2 == 0:
            string = string_after(skip)
            skip = skip + parts[j // 2]
        one = _shr(escapes[j], 3)
        mask = (escapes[j] << 2) - one
        g = codes[j] - one
        for byte in range(4):
            n = (lax.clz(string) + 1) & (_shr(mask, 8 * byte) if byte else mask)
            string = string << n
            g = g + (n << (8 * byte) if byte else n)
        e = top - g
        if extra is not None:
            e = jnp.where(_is_plain(head0), codes[j] | extra[j], e)
        swap = (e ^ _shr(rest[j], 8)) & 0x00FF00FF
        a.append(_rotl(rest[j] ^ (swap << 8), 31))
        b.append(_rotl(e ^ swap, 31))
    return a + b


def _pieces(block):
    return [block[i:i + 16, j:j + 128] for i in (0, 16) for j in range(0, 1024, 128)]


def _joined(pieces):
    return jnp.concatenate(
        [jnp.concatenate(pieces[:8], axis=1), jnp.concatenate(pieces[8:], axis=1)], axis=0)


def _add(u, v):
    return [a + b for a, b in zip(u, v)]


def _read_tiles(msg, row, count):
    return [msg[row + 8 * j:row + 8 * j + 8, :] for j in range(count)]


def _write_tiles(msg, row, tiles):
    for j, t in enumerate(tiles):
        msg[row + 8 * j:row + 8 * j + 8, :] = t


def _header(msg, k=0):
    return jnp.broadcast_to(msg[HEAD_AT + k:HEAD_AT + k + 1, :], TILE)


def _write_message(msg, pieces):
    main, exps = _encode([pltpu.bitcast(p.astype(BF16), I32) for p in pieces])
    _write_tiles(msg, 0, main)
    _write_tiles(msg, EXTRA_AT, exps)


def _read_message(msg, with_extra):
    extra = _unpack_extra(_read_tiles(msg, EXTRA_AT, 5)) if with_extra else None
    words = _decode(
        _read_tiles(msg, 0, 8), _read_tiles(msg, 64, 3), _header(msg, 0), _header(msg, 1), extra)
    return [pltpu.bitcast(w, BF16).astype(F32) for w in words]


def _needs_extra(msgs):
    sublane = lax.broadcasted_iota(I32, TILE, 0)
    bits = jnp.zeros(TILE, F32)
    for k, msg in enumerate(msgs):
        bits = jnp.where((sublane == k) & _is_plain(_header(msg)), float(1 << k), bits)
    bits = jnp.sum(jnp.max(bits, axis=1, keepdims=True), axis=0, keepdims=True)
    return bits.astype(I32)[0, 0]


class _Message:
    def __init__(self, src, dst, peer, main_sems, extra_sems):
        self.src, self.dst, self.peer = src, dst, peer
        self.main_sems, self.extra_sems = main_sems, extra_sems

    def _copy(self, part, sems):
        return pltpu.make_async_remote_copy(
            self.src.at[part], self.dst.at[part], *sems, **self.peer)

    def main(self):
        return self._copy(pl.ds(0, MAIN_ROWS), self.main_sems)

    def extra(self):
        return self._copy(pl.ds(EXTRA_AT, EXTRA_ROWS), self.extra_sems)

    def send_extra(self):
        _write_tiles(self.src, EXTRA_AT, _pack_extra(_read_tiles(self.src, EXTRA_AT, 8)))
        self.extra().start()

    def receive(self, use):
        self.main().wait_recv()
        return self.unpack(use)

    def unpack(self, use):
        more = _needs_extra([self.dst])
        use(_read_message(self.dst, False))

        @pl.when(more != 0)
        def _():
            self.extra().wait_recv()
            use(_read_message(self.dst, True))

        return more


def _body(x_ref, o_ref, block, send, recv, gathered, gathered_more,
          load_sem, main_sem, extra_sem, sent_main_sem, sent_extra_sem, entered):
    n, _, cols = block.shape
    first_raw = n - RAW
    mx, my = lax.axis_index("x"), lax.axis_index("y")
    mine = pl.ds(pl.multiple_of(my * cols, cols), cols)
    other = pl.ds(pl.multiple_of((1 - my) * cols, cols), cols)

    def peer(link):
        return dict(device_id=(mx ^ link ^ 1, my ^ link), device_id_type=pl.DeviceIdType.MESH)

    def rows(c):
        return pl.ds(c * ROWS if isinstance(c, int) else pl.multiple_of(c * ROWS, ROWS), ROWS)

    def load(c):
        return pltpu.make_async_copy(x_ref.at[0, rows(c)], block.at[c], load_sem.at[c])

    def store(c, where, pieces):
        o_ref[rows(c), where] = _joined(pieces).astype(BF16)

    def message(link, c, src):
        sem = link * (n + RAW) + c
        return _Message(src, recv.at[link, c], peer(link),
                        (sent_main_sem.at[link], main_sem.at[sem]),
                        (sent_extra_sem, extra_sem.at[sem]))

    def streamed(link, c):
        return message(link, c, send.at[link, c])

    def gather(k):
        return message(1, first_raw + k, send.at[0, first_raw + k])

    def pass_on(k):
        return message(0, n + k, gather(k).dst)

    def pass_on_part(link):
        where = pl.ds(VIA_X, MAIN_ROWS - VIA_X) if link else pl.ds(0, VIA_X)
        return pltpu.make_async_remote_copy(
            recv.at[1 - link, first_raw, where], recv.at[0, n, where],
            sent_main_sem.at[2 + link], main_sem.at[link * (n + RAW) + n], **peer(link))

    load(0).start()

    barrier = pltpu.get_barrier_semaphore()
    starts_last, not_held_up = (mx == 1) & (my == 1), (mx == 1) & (my == 0)
    pl.semaphore_signal(barrier, inc=1, **peer(0))
    pl.when(~starts_last)(lambda: pl.semaphore_signal(barrier, inc=1, **peer(1)))

    @pl.when(starts_last)
    def _():
        pl.semaphore_wait(barrier, 2)
        pl.semaphore_signal(entered, inc=1, **peer(1))

    def opening(t):
        link = t & 1
        c = (t >> 1) + link * first_raw
        return c, message(link, c, send.at[0, c])

    @pl.loop(0, AHEAD + RAW)
    def _(t):
        c, msg = opening(t)
        load(c).wait()

        @pl.when(t == 0)
        def _():
            for later in range(1, AHEAD + RAW):
                load(opening(later)[0]).start()
            for later in range(AHEAD, AHEAD + LOADS):
                load(later).start()

        _write_message(msg.src, _pieces(block.at[c]))
        pl.when((t == 0) & (mx == 0))(lambda: pl.semaphore_wait(barrier, 2))
        pl.when((t == 0) & not_held_up)(lambda: pl.semaphore_wait(barrier, 1))
        pl.when((t == 1) & not_held_up)(lambda: pl.semaphore_wait(entered, 1))
        msg.main().start()

    opening_more = _needs_extra([opening(t)[1].src for t in range(AHEAD + RAW)])

    def opening_extra(t, extras):
        more = (opening_more >> t) & 1
        pl.when(more != 0)(opening(t)[1].send_extra)
        return extras + more

    extras = lax.fori_loop(0, AHEAD + RAW, opening_extra, 0)

    def raw_more(k):
        return (opening_more >> (2 * k + 1)) & 1

    def step(i, extras):
        unpacking = i >= LAG
        j = jnp.maximum(i - LAG, 0)
        addend, summed, theirs = streamed(0, i), streamed(1, i), streamed(1, j)
        sent_x = streamed(0, jnp.minimum(i + AHEAD - 1, first_raw - 1))
        sent_y = streamed(1, jnp.maximum(i - 1, 0))

        pl.when(unpacking)(lambda: theirs.main().wait_recv())
        addend.main().wait_recv()
        more = _needs_extra([
            addend.dst,
            recv.at[unpacking.astype(I32), jnp.where(unpacking, j, i)],
            sent_x.src,
            send.at[(i > 0).astype(I32), jnp.maximum(i - 1, 0)],
        ])
        more_x = ((more & 4) != 0) & (i > 0) & (i + AHEAD - 1 < first_raw)
        more_y = ((more & 8) != 0) & (i > 0)

        def add(with_extra):
            total = _add(_pieces(block.at[i]), _read_message(addend.dst, with_extra))
            _write_message(summed.src, total)
            store(i, mine, total)

        add(False)

        @pl.when(more != 0)
        def _():
            pl.when(more_x)(sent_x.send_extra)
            pl.when(more_y)(sent_y.send_extra)

            @pl.when((more & 1) != 0)
            def _():
                addend.extra().wait_recv()
                add(True)

        summed.main().start()

        c = i + AHEAD

        @pl.when(c < first_raw)
        def _():
            load(c).wait()
            _write_message(send.at[0, c], _pieces(block.at[c]))
            streamed(0, c).main().start()
            pl.when(c + LOADS < first_raw)(lambda: load(c + LOADS).start())

        @pl.when((c >= first_raw) & (c < n))
        def _():
            streamed(0, c).main().start()
            pl.when(raw_more(c - first_raw) != 0)(lambda: streamed(0, c).extra().start())

        @pl.when(c == n)
        def _():
            pass_on(1).main().start()
            pl.when(gathered_more[1] != 0)(lambda: pass_on(1).extra().start())
            pass_on_part(0).start()
            pl.when(gathered_more[0] != 0)(lambda: pass_on(0).extra().start())

        @pl.when((i >= LAG - RAW) & (i < LAG))
        def _():
            k = i - (LAG - RAW)

            def keep(pieces):
                gathered[k] = _joined(pieces)

            gathered_more[k] = gather(k).receive(keep)

        @pl.when(unpacking)
        def _():
            store(j, other, _read_message(theirs.dst, False))

            @pl.when((more & 2) != 0)
            def _():
                theirs.extra().wait_recv()
                store(j, other, _read_message(theirs.dst, True))

        return extras + more_x.astype(I32) + more_y.astype(I32)

    extras = lax.fori_loop(0, first_raw, step, extras)
    final = streamed(1, first_raw - 1)
    more = _needs_extra([final.src])
    pl.when(more != 0)(final.send_extra)
    extras = extras + more + sum(raw_more(k) + gathered_more[k] for k in range(RAW))

    @pl.loop(first_raw - LAG, first_raw)
    def _(j):
        streamed(1, j).receive(lambda v: store(j, other, v))
        c = j + LAG

        @pl.when(c < n)
        def _():
            addend = streamed(0, c)
            addend.main().wait_recv()
            pl.when(c == first_raw)(lambda: pass_on_part(1).start())
            addend.unpack(lambda v: store(c, mine, _add(_pieces(block.at[c]), v)))

    @pl.loop(0, RAW)
    def _(t):
        k = RAW - 1 - t
        pl.when(k > 0)(lambda: pass_on(k).main().wait_recv())

        @pl.when(k == 0)
        def _():
            pass_on_part(0).wait()
            pass_on_part(1).wait()

        pass_on(k).unpack(lambda v: store(first_raw + k, other, _add(_pieces(gathered.at[k]), v)))

    def wait_sent(like, sem):
        pltpu.make_async_remote_copy(like, like, sem, sem, **peer(0)).wait_send()

    wait_sent(send.at[0, pl.ds(0, n + 1), pl.ds(0, MAIN_ROWS)], sent_main_sem.at[0])
    wait_sent(send.at[1, pl.ds(0, n), pl.ds(0, MAIN_ROWS)], sent_main_sem.at[1])

    @pl.loop(0, extras)
    def _(_):
        wait_sent(send.at[0, 0, pl.ds(EXTRA_AT, EXTRA_ROWS)], sent_extra_sem)


def pallas_dist_rsx_agy_m2048_n1024_kernel(x: jax.Array):
    _, m, cols = x.shape
    n = m // ROWS
    messages = pltpu.VMEM((2, n + RAW, SLOT_ROWS, 128), I32)
    return pl.pallas_call(
        _body,
        out_shape=jax.ShapeDtypeStruct((m, 2 * cols), BF16),
        in_specs=[pl.BlockSpec(memory_space=pltpu.HBM)],
        out_specs=pl.BlockSpec(memory_space=pltpu.VMEM),
        scratch_shapes=[
            pltpu.VMEM((n, ROWS, cols), F32),
            messages,
            messages,
            pltpu.VMEM((RAW, ROWS, cols), F32),
            pltpu.SMEM((RAW,), I32),
            pltpu.SemaphoreType.DMA((n,)),
            pltpu.SemaphoreType.DMA((2 * (n + RAW),)),
            pltpu.SemaphoreType.DMA((2 * (n + RAW),)),
            pltpu.SemaphoreType.DMA((4,)),
            pltpu.SemaphoreType.DMA,
            pltpu.SemaphoreType.REGULAR,
        ],
        compiler_params=pltpu.CompilerParams(
            collective_id=0, vmem_limit_bytes=40 << 20, disable_semaphore_checks=True),
        name="rsx_agy",
    )(x)
```
